```python
import numpy as np

kernel_name = "dist_moe_cap_ep_outshard_n2048_d512_e8_h1024"

def setup_inputs():
    x = np.random.randn(2048, 512).astype(np.float32)
    router_W = np.random.randn(512, 32).astype(np.float32) * 0.1
    scores64 = x.astype(np.float64) @ router_W.astype(np.float64)
    route_idx = np.argsort(-scores64, axis=-1)[:, :1].astype(np.int32)
    expert_W = np.random.randn(32, 512, 1024).astype(np.float32) * 0.02
    return {"x": x, "router_W": router_W, "route_idx": route_idx, "expert_W": expert_W}

def reference(x, router_W, route_idx, expert_W):
    counts = np.zeros(32, dtype=np.int64)
    out = np.zeros((2048, 1024), dtype=np.float32)
    for i in range(2048):
        e = int(route_idx[i, 0])
        if counts[e] < 51:
            out[i] = x[i] @ expert_W[e]
            counts[e] += 1
    return out
```

```python
import jax
import jax.numpy as jnp
from jax import lax
from jax.experimental import pallas as pl
from jax.experimental.pallas import tpu as pltpu

N_DEV = 4
N_TOK = 2048
D = 512
H = 1024
E_LOC = 8
N_EXP = 32
CAP = 51
SLOT = 64
ROWS_PER_DEV = N_TOK // N_DEV
BF = jnp.bfloat16
F32 = jnp.float32
I32 = jnp.int32
PROFILE = False
RECV_AFTER = {2: (0,), 3: (1,), 4: (2,), 5: (3,), 6: (4, 5), 7: (6, 7)}

T_RANK = 0
T_BND = 16
T_TOK = 18
T_DST = 22
T_SRC = 26
T_ROWS = 32


def _iota(shape, dim):
    return lax.broadcasted_iota(I32, shape, dim)


def _dot(a, b):
    return jnp.dot(a, b, preferred_element_type=F32)


def _dot_nt(a, b):
    return lax.dot_general(a, b, (((1,), (1,)), ((), ())), preferred_element_type=F32)


def _row512(a4):
    return jnp.concatenate([a4[k:k + 1, :] for k in range(4)], axis=1)


class _scope:
    def __init__(self, name):
        self.s = jax.named_scope(name) if PROFILE else None

    def __enter__(self):
        if self.s is not None:
            self.s.__enter__()

    def __exit__(self, *a):
        if self.s is not None:
            self.s.__exit__(*a)


def _body(r_ref, x_hbm, w_hbm, obuf,
          wbuf, xg, st, tab_v, tab_s,
          wsem, gsem, tsem, send_sem, recv_sem, sem2):
    me = lax.axis_index("i")

    def wcopy(j):
        return pltpu.make_async_copy(w_hbm.at[j], wbuf.at[j], wsem.at[j])

    for j in range(E_LOC):
        wcopy(j).start(priority=1)

    barrier = pltpu.get_barrier_semaphore()
    for k in range(1, N_DEV):
        pl.semaphore_signal(barrier, inc=1, device_id=((me + k) % N_DEV,),
                            device_id_type=pl.DeviceIdType.MESH)

    with _scope("routing"):
        r2 = r_ref[...]
        ones_b = jnp.ones((128, 128), BF)
        ones8 = jnp.ones((8, 128), BF)
        utri = (_iota((128, 128), 0) <= _iota((128, 128), 1)).astype(BF)

        rl = jnp.concatenate([r2] * E_LOC, axis=0)
        ohl = (rl == (me * E_LOC + (_iota((128, 128), 0) >> 4))).astype(BF)
        c_in_l = _dot(ohl, utri)
        tot_bl = _dot(ohl, ones_b)
        li = _iota((128, 128), 0)
        lj = _iota((128, 128), 1)
        lblk_l = (((li >> 4) == (lj >> 4)) & ((lj & 15) < (li & 15))).astype(BF)
        pre_l = jnp.minimum(_dot(lblk_l, tot_bl.astype(BF)), 64.0)
        tot_row_l = _dot_nt(ones8, ohl)
        pre_row_l = _dot_nt(tot_row_l.astype(BF), lblk_l)
        pr = pre_row_l[0:1, :]
        br = pr + tot_row_l[0:1, :]
        pi = _iota((512, 128), 0)
        pj = _iota((512, 128), 1)
        cf = (pi & 63).astype(F32)
        onehot = (((pi >> 6) == (pj >> 4)) & (pr <= cf) & (br > cf)).astype(BF)
        g = _dot(onehot, c_in_l.astype(BF))
        presel = _dot(onehot, pre_l.astype(BF))
        cmp_b = (g <= cf - presel).astype(BF)
        l_row = _dot_nt(ones8, cmp_b)
        bvec = (_iota((8, 128), 1) & 15).astype(BF)
        b_row = _dot_nt(bvec, onehot)
        tok_row = (b_row * 128.0 + l_row).astype(I32)
        for k in range(4):
            tab_v[T_TOK + k:T_TOK + k + 1, :] = tok_row[0:1, 128 * k:128 * (k + 1)]

        rt = jnp.concatenate([r2] * N_EXP, axis=0)
        oh = (rt == (_iota((512, 128), 0) >> 4))
        oh_f = oh.astype(F32)
        oh_b = oh.astype(BF)
        c_in = _dot(oh_b, utri)
        tot_b = _dot(oh_b, ones_b)
        qi = _iota((512, 512), 0)
        qj = _iota((512, 512), 1)
        lblk = (((qi >> 4) == (qj >> 4)) & ((qj & 15) < (qi & 15))).astype(BF)
        pre = _dot(lblk, tot_b.astype(BF))
        rank = (oh_f * (c_in + pre - 1.0)).reshape(N_EXP, 16, 128).sum(axis=0)
        tab_v[T_RANK:T_RANK + 16, :] = rank.astype(I32)

        tot_row = _dot_nt(ones8, oh_b)
        mi = _iota((512, 256), 0)
        mj = _iota((512, 256), 1)
        m_b = (((mi >> 4) == (mj >> 3)) & ((mi & 15) < 4 * (mj & 7))).astype(BF)
        bnd = jnp.minimum(_dot(tot_row.astype(BF), m_b), float(CAP)).astype(I32)
        tab_v[T_BND:T_BND + 1, :] = bnd[0:1, 0:128]
        tab_v[T_BND + 1:T_BND + 2, :] = bnd[0:1, 128:256]

        my_r = r_ref[pl.ds(4 * me, 4), :]
        my_rank = tab_v[pl.ds(T_RANK + 4 * me, 4), :]
        cls = jnp.where(my_rank < CAP, my_r & 7, 8)
        ct = jnp.concatenate([cls] * 10, axis=0)
        ohc = (ct == (_iota((40, 128), 0) >> 2))
        ohc_b = ohc.astype(BF)
        cc_in = _dot(ohc_b, utri)
        ctot = _dot(ohc_b, ones_b)
        ci = _iota((40, 40), 0)
        cj = _iota((40, 40), 1)
        lfull = (((cj >> 2) < (ci >> 2)) | (((cj >> 2) == (ci >> 2)) & ((cj & 3) < (ci & 3)))).astype(BF)
        cpre = _dot(lfull, ctot.astype(BF))
        pos = (ohc.astype(F32) * (cc_in + cpre - 1.0)).reshape(10, 4, 128).sum(axis=0)
        pos_row = _row512(pos.astype(I32))
        mp = (_iota((512, 512), 0) == pos_row).astype(BF)
        lane = _iota((1, 512), 1)
        vals = jnp.concatenate([
            (lane & 127).astype(F32),
            (lane >> 7).astype(F32),
            _row512(my_r).astype(F32),
            _row512(jnp.minimum(my_rank, 63)).astype(F32),
            jnp.zeros((4, 512), F32)], axis=0).astype(BF)
        res = _dot_nt(vals, mp).astype(I32)
        irow = res[1:2, :] * 128 + res[0:1, :]
        dst_row = (irow >> 3) * 64 + (irow & 7)
        src_row = res[2:3, :] * SLOT + res[3:4, :]
        for k in range(4):
            tab_v[T_DST + k:T_DST + k + 1, :] = dst_row[:, 128 * k:128 * (k + 1)]
            tab_v[T_SRC + k:T_SRC + k + 1, :] = src_row[:, 128 * k:128 * (k + 1)]
        tab_v[T_SRC + 4:T_ROWS, :] = jnp.zeros((T_ROWS - T_SRC - 4, 128), I32)

    with _scope("tabdma"):
        tcp = pltpu.make_async_copy(tab_v, tab_s, tsem)
        tcp.start()
        pl.semaphore_wait(barrier, N_DEV - 1)
        for k in range(1, N_DEV):
            pl.semaphore_signal(sem2, inc=1, device_id=((me + k) % N_DEV,),
                                device_id_type=pl.DeviceIdType.MESH)
        tcp.wait()

    def tab(row0, idx):
        return tab_s[row0 + (idx >> 7), idx & 127]

    def bnd_s(e, d):
        return tab(T_BND, e * 8 + d)

    def gather(j):
        def one(c, carry):
            t = tab(T_TOK, j * SLOT + c)
            pltpu.make_async_copy(x_hbm.at[pl.ds(t, 1)], xg.at[j, pl.ds(c, 1)], gsem.at[j]).start()
            return carry
        lax.fori_loop(0, CAP, one, 0)

    def seg_copy(e, d, owner):
        a = bnd_s(e, d)
        n = bnd_s(e, d + 1) - a
        sl = st.at[pl.ds(e * SLOT + a, n)]
        jloc = e - owner * E_LOC
        cp = pltpu.make_async_remote_copy(
            src_ref=sl, dst_ref=sl,
            send_sem=send_sem.at[jloc * N_DEV + d], recv_sem=recv_sem.at[e],
            device_id=(d,), device_id_type=pl.DeviceIdType.MESH)
        return n, cp

    def compute(j):
        e = me * E_LOC + j
        wcopy(j).wait()
        sl = xg.at[j, pl.ds(0, 48)]
        pltpu.make_async_copy(sl, sl, gsem.at[j]).wait()
        for c in range(48, CAP):
            sl = xg.at[j, pl.ds(c, 1)]
            pltpu.make_async_copy(sl, sl, gsem.at[j]).wait()
        xb = xg[j].astype(BF)
        y = _dot(xb, wbuf[j].astype(BF))
        yr = pltpu.bitcast(y.astype(BF).astype(F32), I32)
        u = yr[:, :512] | lax.shift_right_logical(yr[:, 512:], 16)
        base = pl.multiple_of(e * SLOT, SLOT)
        for c in range(4):
            st[pl.ds(base, SLOT), c, :] = u[:, c * 128:(c + 1) * 128]
        if j == 0:
            pl.semaphore_wait(sem2, N_DEV - 1)
        for k in range(1, N_DEV):
            d = (me + k) % N_DEV
            n, cp = seg_copy(e, d, me)

            @pl.when(n > 0)
            def _():
                cp.start()

    def receive(j, off):
        cnt = 0
        for s_ in range(N_DEV):
            e = s_ * E_LOC + j
            cnt = cnt + bnd_s(e, me + 1) - bnd_s(e, me)
        for k in range(1, N_DEV):
            s_ = (me + k) % N_DEV
            n, cp = seg_copy(s_ * E_LOC + j, me, s_)

            @pl.when(n > 0)
            def _():
                cp.wait_recv()

        def row(p):
            dst = tab(T_DST, p)
            src = tab(T_SRC, p)
            v = st[src]
            obuf[pl.ds(dst, 4, stride=8), :] = pltpu.bitcast(v & jnp.int32(-65536), F32)
            obuf[pl.ds(dst + 32, 4, stride=8), :] = pltpu.bitcast(v << 16, F32)

        def four(q, carry):
            for t in range(4):
                row(off + 4 * q + t)
            return carry

        def one(p, carry):
            row(p)
            return carry
        n4 = cnt >> 2
        lax.fori_loop(0, n4, four, 0)
        lax.fori_loop(off + 4 * n4, off + cnt, one, 0)
        return off + cnt

    with _scope("g0"):
        gather(0)
    with _scope("g1"):
        gather(1)
    with _scope("zero"):
        obuf[...] = jnp.zeros(obuf.shape, F32)
    off = 0
    for j in range(E_LOC):
        with _scope(f"c{j}"):
            compute(j)
        if j + 2 < E_LOC:
            with _scope(f"g{j+2}"):
                gather(j + 2)
        for jr in RECV_AFTER.get(j, ()):
            with _scope(f"r{jr}"):
                off = receive(jr, off)

    with _scope("out"):
        for j in range(E_LOC):
            e = me * E_LOC + j
            for k in range(1, N_DEV):
                d = (me + k) % N_DEV
                n, cp = seg_copy(e, d, me)

                @pl.when(n > 0)
                def _():
                    cp.wait_send()


def pallas_dist_moe_cap_ep_outshard_n2048_d512_e8_h1024_kernel(x, router_W, route_idx, expert_W):
    del router_W
    r2 = route_idx.reshape(16, 128)
    out = pl.pallas_call(
        _body,
        out_shape=jax.ShapeDtypeStruct((ROWS_PER_DEV * 8, 128), F32),
        in_specs=[pl.BlockSpec(memory_space=pltpu.VMEM),
                  pl.BlockSpec(memory_space=pl.ANY),
                  pl.BlockSpec(memory_space=pl.ANY)],
        out_specs=pl.BlockSpec(memory_space=pltpu.VMEM),
        scratch_shapes=[
            pltpu.VMEM((E_LOC, D, H), F32),
            pltpu.VMEM((E_LOC, SLOT, D), F32),
            pltpu.VMEM((N_EXP * SLOT, 4, 128), I32),
            pltpu.VMEM((T_ROWS, 128), I32),
            pltpu.SMEM((T_ROWS, 128), I32),
            pltpu.SemaphoreType.DMA((E_LOC,)),
            pltpu.SemaphoreType.DMA((E_LOC,)),
            pltpu.SemaphoreType.DMA,
            pltpu.SemaphoreType.DMA((E_LOC * N_DEV,)),
            pltpu.SemaphoreType.DMA((N_EXP,)),
            pltpu.SemaphoreType.REGULAR,
        ],
        compiler_params=pltpu.CompilerParams(collective_id=0, vmem_limit_bytes=64 * 1024 * 1024),
    )(r2, x, expert_W)
    return out.reshape(64, 8, 8, 128).transpose(0, 2, 1, 3).reshape(ROWS_PER_DEV, H)
```

```python
import jax
import jax.numpy as jnp
from jax import lax
from jax.experimental import pallas as pl
from jax.experimental.pallas import tpu as pltpu

N_DEV = 4
N_TOK = 2048
D = 512
H = 1024
E_LOC = 8
N_EXP = 32
CAP = 51
SLOT = 64
ROWS_PER_DEV = N_TOK // N_DEV
LAST = E_LOC - 1
NPC = 4
PW = H // NPC
UNR = 4
BF = jnp.bfloat16
F32 = jnp.float32
I32 = jnp.int32
RECV_AFTER = {2: (0,), 3: (1,), 4: (2,), 5: (3,), 6: (4, 5)}

T_RANK = 0
T_BND = 16
T_TOK = 18
T_DST = 22
T_SRC = 26
T_ROWS = 32


def _iota(shape, dim):
    return lax.broadcasted_iota(I32, shape, dim)


def _dot(a, b):
    return jnp.dot(a, b, preferred_element_type=F32)


def _dot_nt(a, b):
    return lax.dot_general(a, b, (((1,), (1,)), ((), ())), preferred_element_type=F32)


def _row512(a4):
    return jnp.concatenate([a4[k:k + 1, :] for k in range(4)], axis=1)


def _routing(me, r_ref, tab_v):
    r2 = r_ref[...]
    ones_b = jnp.ones((128, 128), BF)
    ones8 = jnp.ones((8, 128), BF)
    utri = (_iota((128, 128), 0) <= _iota((128, 128), 1)).astype(BF)

    rl = jnp.concatenate([r2] * E_LOC, axis=0)
    ohl = (rl == (me * E_LOC + (_iota((128, 128), 0) >> 4))).astype(BF)
    c_in_l = _dot(ohl, utri)
    tot_bl = _dot(ohl, ones_b)
    li = _iota((128, 128), 0)
    lj = _iota((128, 128), 1)
    lblk_l = (((li >> 4) == (lj >> 4)) & ((lj & 15) < (li & 15))).astype(BF)
    pre_l = jnp.minimum(_dot(lblk_l, tot_bl.astype(BF)), 64.0)
    tot_row_l = _dot_nt(ones8, ohl)
    pre_row_l = _dot_nt(tot_row_l.astype(BF), lblk_l)
    pr = pre_row_l[0:1, :]
    br = pr + tot_row_l[0:1, :]
    pi = _iota((512, 128), 0)
    pj = _iota((512, 128), 1)
    cf = (pi & 63).astype(F32)
    onehot = (((pi >> 6) == (pj >> 4)) & (pr <= cf) & (br > cf)).astype(BF)
    g = _dot(onehot, c_in_l.astype(BF))
    presel = _dot(onehot, pre_l.astype(BF))
    cmp_b = (g <= cf - presel).astype(BF)
    l_row = _dot_nt(ones8, cmp_b)
    bvec = (_iota((8, 128), 1) & 15).astype(BF)
    b_row = _dot_nt(bvec, onehot)
    tok_row = (b_row * 128.0 + l_row).astype(I32)
    for k in range(4):
        tab_v[T_TOK + k:T_TOK + k + 1, :] = tok_row[0:1, 128 * k:128 * (k + 1)]

    rt = jnp.concatenate([r2] * N_EXP, axis=0)
    oh = (rt == (_iota((512, 128), 0) >> 4))
    oh_f = oh.astype(F32)
    oh_b = oh.astype(BF)
    c_in = _dot(oh_b, utri)
    tot_b = _dot(oh_b, ones_b)
    qi = _iota((512, 512), 0)
    qj = _iota((512, 512), 1)
    lblk = (((qi >> 4) == (qj >> 4)) & ((qj & 15) < (qi & 15))).astype(BF)
    pre = _dot(lblk, tot_b.astype(BF))
    rank = (oh_f * (c_in + pre - 1.0)).reshape(N_EXP, 16, 128).sum(axis=0)
    tab_v[T_RANK:T_RANK + 16, :] = rank.astype(I32)

    tot_row = _dot_nt(ones8, oh_b)
    mi = _iota((512, 256), 0)
    mj = _iota((512, 256), 1)
    m_b = (((mi >> 4) == (mj >> 3)) & ((mi & 15) < 4 * (mj & 7))).astype(BF)
    bnd = jnp.minimum(_dot(tot_row.astype(BF), m_b), float(CAP)).astype(I32)
    tab_v[T_BND:T_BND + 1, :] = bnd[0:1, 0:128]
    tab_v[T_BND + 1:T_BND + 2, :] = bnd[0:1, 128:256]

    my_r = r_ref[pl.ds(4 * me, 4), :]
    my_rank = tab_v[pl.ds(T_RANK + 4 * me, 4), :]
    cls = jnp.where(my_rank < CAP, my_r & 7, 8)
    ct = jnp.concatenate([cls] * 10, axis=0)
    ohc = (ct == (_iota((40, 128), 0) >> 2))
    ohc_b = ohc.astype(BF)
    cc_in = _dot(ohc_b, utri)
    ctot = _dot(ohc_b, ones_b)
    ci = _iota((40, 40), 0)
    cj = _iota((40, 40), 1)
    lfull = (((cj >> 2) < (ci >> 2))
             | (((cj >> 2) == (ci >> 2)) & ((cj & 3) < (ci & 3)))).astype(BF)
    cpre = _dot(lfull, ctot.astype(BF))
    pos = (ohc.astype(F32) * (cc_in + cpre - 1.0)).reshape(10, 4, 128).sum(axis=0)
    pos_row = _row512(pos.astype(I32))
    mp = (_iota((512, 512), 0) == pos_row).astype(BF)
    lane = _iota((1, 512), 1)
    vals = jnp.concatenate([
        (lane & 127).astype(F32),
        (lane >> 7).astype(F32),
        _row512(my_r).astype(F32),
        _row512(jnp.minimum(my_rank, SLOT - 1)).astype(F32),
        jnp.zeros((4, 512), F32)], axis=0).astype(BF)
    res = _dot_nt(vals, mp).astype(I32)
    irow = res[1:2, :] * 128 + res[0:1, :]
    dst_row = (irow >> 3) * 64 + (irow & 7)
    src_row = res[2:3, :] * SLOT + res[3:4, :]
    for k in range(4):
        tab_v[T_DST + k:T_DST + k + 1, :] = dst_row[:, 128 * k:128 * (k + 1)]
        tab_v[T_SRC + k:T_SRC + k + 1, :] = src_row[:, 128 * k:128 * (k + 1)]
    tab_v[T_SRC + 4:T_ROWS, :] = jnp.zeros((T_ROWS - T_SRC - 4, 128), I32)


def _body(r_hbm, x_hbm, w_hbm, obuf,
          wbuf, xg, st, st7, r_ref, tab_v, tab_s,
          wsem, wsem7, gsem, tsem, send_sem, recv_sem, send7, recv7, sem2):
    me = lax.axis_index("i")

    def wcopy(j):
        return pltpu.make_async_copy(w_hbm.at[j], wbuf.at[j], wsem.at[j])

    def wcopy7(q):
        return pltpu.make_async_copy(w_hbm.at[LAST, :, pl.ds(q * PW, PW)],
                                     wbuf.at[LAST, :, pl.ds(q * PW, PW)], wsem7.at[q])

    rcp = pltpu.make_async_copy(r_hbm, r_ref, tsem)
    rcp.start()
    for j in range(LAST):
        wcopy(j).start(priority=1)
    for q in range(NPC):
        wcopy7(q).start(priority=1)

    barrier = pltpu.get_barrier_semaphore()
    for k in range(1, N_DEV):
        pl.semaphore_signal(barrier, inc=1, device_id=((me + k) % N_DEV,),
                            device_id_type=pl.DeviceIdType.MESH)

    rcp.wait()
    _routing(me, r_ref, tab_v)

    tcp = pltpu.make_async_copy(tab_v, tab_s, tsem)
    tcp.start()
    pl.semaphore_wait(barrier, N_DEV - 1)
    for k in range(1, N_DEV):
        pl.semaphore_signal(sem2, inc=1, device_id=((me + k) % N_DEV,),
                            device_id_type=pl.DeviceIdType.MESH)
    tcp.wait()

    def tab(row0, idx):
        return tab_s[row0 + (idx >> 7), idx & 127]

    def bnd_s(e, d):
        return tab(T_BND, e * 8 + d)

    def gather(j):
        def one(c, carry):
            t = tab(T_TOK, j * SLOT + c)
            pltpu.make_async_copy(x_hbm.at[pl.ds(t, 1)], xg.at[j, pl.ds(c, 1)], gsem.at[j]).start()
            return carry
        lax.fori_loop(0, CAP, one, 0)

    def gather_wait(j):
        sl = xg.at[j, pl.ds(0, 48)]
        pltpu.make_async_copy(sl, sl, gsem.at[j]).wait()
        for c in range(48, CAP):
            sl = xg.at[j, pl.ds(c, 1)]
            pltpu.make_async_copy(sl, sl, gsem.at[j]).wait()

    def seg_copy(e, d, owner):
        a = bnd_s(e, d)
        n = bnd_s(e, d + 1) - a
        sl = st.at[pl.ds(e * SLOT + a, n)]
        jloc = e - owner * E_LOC
        cp = pltpu.make_async_remote_copy(
            src_ref=sl, dst_ref=sl,
            send_sem=send_sem.at[jloc * N_DEV + d], recv_sem=recv_sem.at[e],
            device_id=(d,), device_id_type=pl.DeviceIdType.MESH)
        return n, cp

    def seg7(q, d, owner):
        e = owner * E_LOC + LAST
        a = bnd_s(e, d)
        n = bnd_s(e, d + 1) - a
        sl = st7.at[pl.ds((q * N_DEV + owner) * SLOT + a, n)]
        cp = pltpu.make_async_remote_copy(
            src_ref=sl, dst_ref=sl,
            send_sem=send7.at[q * N_DEV + d], recv_sem=recv7.at[q * N_DEV + owner],
            device_id=(d,), device_id_type=pl.DeviceIdType.MESH)
        return n, cp

    def compute(j):
        e = me * E_LOC + j
        wcopy(j).wait()
        gather_wait(j)
        xb = xg[j].astype(BF)
        y = _dot(xb, wbuf[j].astype(BF))
        yr = pltpu.bitcast(y.astype(BF).astype(F32), I32)
        base = pl.multiple_of(e * SLOT, SLOT)
        for c in range(4):
            st[pl.ds(base, SLOT), c, :] = (
                yr[:, 256 * c:256 * c + 128]
                | lax.shift_right_logical(yr[:, 256 * c + 128:256 * c + 256], 16))
        if j == 0:
            pl.semaphore_wait(sem2, N_DEV - 1)
        for k in range(1, N_DEV):
            d = (me + k) % N_DEV
            n, cp = seg_copy(e, d, me)

            @pl.when(n > 0)
            def _():
                cp.start()

    def compute7():
        gather_wait(LAST)
        xb = xg[LAST].astype(BF)
        for q in range(NPC):
            wcopy7(q).wait()
            y = _dot(xb, wbuf[LAST, :, q * PW:(q + 1) * PW].astype(BF))
            yr = pltpu.bitcast(y.astype(BF).astype(F32), I32)
            base = pl.multiple_of((q * N_DEV + me) * SLOT, SLOT)
            st7[pl.ds(base, SLOT), 0, :] = yr[:, :128] | lax.shift_right_logical(yr[:, 128:], 16)
            for k in range(1, N_DEV):
                d = (me + k) % N_DEV
                n, cp = seg7(q, d, me)

                @pl.when(n > 0)
                def _():
                    cp.start()

    def step_count(j):
        cnt = 0
        for s_ in range(N_DEV):
            e = s_ * E_LOC + j
            cnt = cnt + bnd_s(e, me + 1) - bnd_s(e, me)
        return cnt

    def place(off, cnt, load):
        def row(p):
            dst = tab(T_DST, p)
            v = load(tab(T_SRC, p))
            obuf[pl.ds(dst, 4, stride=16), :] = pltpu.bitcast(v & jnp.int32(-65536), F32)
            obuf[pl.ds(dst + 8, 4, stride=16), :] = pltpu.bitcast(v << 16, F32)

        def group(g_, carry):
            for t in range(UNR):
                row(off + UNR * g_ + t)
            return carry

        def one(p, carry):
            row(p)
            return carry
        ng = cnt // UNR
        lax.fori_loop(0, ng, group, 0)
        lax.fori_loop(off + UNR * ng, off + cnt, one, 0)

    def receive(j, off):
        cnt = step_count(j)
        for k in range(1, N_DEV):
            s_ = (me + k) % N_DEV
            n, cp = seg_copy(s_ * E_LOC + j, me, s_)

            @pl.when(n > 0)
            def _():
                cp.wait_recv()
        place(off, cnt, lambda src: st[src])
        return off + cnt

    def receive7(off):
        cnt = step_count(LAST)
        for q in range(NPC):
            for k in range(1, N_DEV):
                s_ = (me + k) % N_DEV
                n, cp = seg7(q, me, s_)

                @pl.when(n > 0)
                def _():
                    cp.wait_recv()

        def load(src):
            slot = (src >> 9) * SLOT + (src & (SLOT - 1))
            return st7[pl.ds(slot, NPC, stride=N_DEV * SLOT), 0, :]
        place(off, cnt, load)

    gather(0)
    gather(1)
    obuf[...] = jnp.zeros(obuf.shape, F32)
    off = 0
    for j in range(LAST):
        compute(j)
        if j + 2 < E_LOC:
            gather(j + 2)
        for jr in RECV_AFTER.get(j, ()):
            off = receive(jr, off)
    compute7()
    off = receive(LAST - 1, off)

    for j in range(LAST):
        for k in range(1, N_DEV):
            d = (me + k) % N_DEV
            n, cp = seg_copy(me * E_LOC + j, d, me)

            @pl.when(n > 0)
            def _():
                cp.wait_send()
    for q in range(NPC):
        for k in range(1, N_DEV):
            d = (me + k) % N_DEV
            n, cp = seg7(q, d, me)

            @pl.when(n > 0)
            def _():
                cp.wait_send()
    receive7(off)


def pallas_dist_moe_cap_ep_outshard_n2048_d512_e8_h1024_kernel(x, router_W, route_idx, expert_W):
    del router_W
    r2 = route_idx.reshape(16, 128)
    out = pl.pallas_call(
        _body,
        out_shape=jax.ShapeDtypeStruct((ROWS_PER_DEV * 8, 128), F32),
        in_specs=[pl.BlockSpec(memory_space=pl.ANY),
                  pl.BlockSpec(memory_space=pl.ANY),
                  pl.BlockSpec(memory_space=pl.ANY)],
        out_specs=pl.BlockSpec(memory_space=pltpu.VMEM),
        scratch_shapes=[
            pltpu.VMEM((E_LOC, D, H), F32),
            pltpu.VMEM((E_LOC, SLOT, D), F32),
            pltpu.VMEM((N_EXP * SLOT, 4, 128), I32),
            pltpu.VMEM((NPC * N_DEV * SLOT, 1, 128), I32),
            pltpu.VMEM((16, 128), I32),
            pltpu.VMEM((T_ROWS, 128), I32),
            pltpu.SMEM((T_ROWS, 128), I32),
            pltpu.SemaphoreType.DMA((E_LOC,)),
            pltpu.SemaphoreType.DMA((NPC,)),
            pltpu.SemaphoreType.DMA((E_LOC,)),
            pltpu.SemaphoreType.DMA,
            pltpu.SemaphoreType.DMA((E_LOC * N_DEV,)),
            pltpu.SemaphoreType.DMA((N_EXP,)),
            pltpu.SemaphoreType.DMA((NPC * N_DEV,)),
            pltpu.SemaphoreType.DMA((NPC * N_DEV,)),
            pltpu.SemaphoreType.REGULAR,
        ],
        compiler_params=pltpu.CompilerParams(
            collective_id=0, vmem_limit_bytes=64 * 1024 * 1024,
            disable_bounds_checks=True, disable_semaphore_checks=True),
    )(r2, x, expert_W)
    return out.reshape(64, 8, 8, 128).transpose(0, 2, 1, 3).reshape(ROWS_PER_DEV, H)
```

```python
import jax
import jax.numpy as jnp
from jax import lax
from jax.experimental import pallas as pl
from jax.experimental.pallas import tpu as pltpu

N_DEV = 4
N_TOK = 2048
D = 512
H = 1024
E_LOC = 8
N_EXP = 32
CAP = 51
SLOT = 64
ROWS_PER_DEV = N_TOK // N_DEV
LAST = E_LOC - 1
NPC = 4
PW = H // NPC
N_CLS = 12
UNR = 4
BF = jnp.bfloat16
F32 = jnp.float32
I32 = jnp.int32
RECV_AFTER = {2: (0,), 3: (1,), 4: (2,), 5: (3,), 6: (4, 5)}

T_RANK = 0
T_BND = 16
T_TOK = 18
T_DST = 22
T_SRC = 26
T_ROWS = 32


def _iota(shape, dim):
    return lax.broadcasted_iota(I32, shape, dim)


def _dot(a, b):
    return jnp.dot(a, b, preferred_element_type=F32)


def _dot_nt(a, b):
    return lax.dot_general(a, b, (((1,), (1,)), ((), ())), preferred_element_type=F32)


def _row512(a4):
    return jnp.concatenate([a4[k:k + 1, :] for k in range(4)], axis=1)


def _routing(me, r_ref, tab_v):
    r2 = r_ref[...]
    ones_b = jnp.ones((128, 128), BF)
    ones8 = jnp.ones((8, 128), BF)
    utri = (_iota((128, 128), 0) <= _iota((128, 128), 1)).astype(BF)

    rl = jnp.concatenate([r2] * E_LOC, axis=0)
    ohl = (rl == (me * E_LOC + (_iota((128, 128), 0) >> 4))).astype(BF)
    c_in_l = _dot(ohl, utri)
    tot_bl = _dot(ohl, ones_b)
    li = _iota((128, 128), 0)
    lj = _iota((128, 128), 1)
    lblk_l = (((li >> 4) == (lj >> 4)) & ((lj & 15) < (li & 15))).astype(BF)
    pre_l = jnp.minimum(_dot(lblk_l, tot_bl.astype(BF)), 64.0)
    tot_row_l = _dot_nt(ones8, ohl)
    pre_row_l = _dot_nt(tot_row_l.astype(BF), lblk_l)
    pr = pre_row_l[0:1, :]
    br = pr + tot_row_l[0:1, :]
    pi = _iota((512, 128), 0)
    pj = _iota((512, 128), 1)
    cf = (pi & 63).astype(F32)
    onehot = (((pi >> 6) == (pj >> 4)) & (pr <= cf) & (br > cf)).astype(BF)
    g = _dot(onehot, c_in_l.astype(BF))
    presel = _dot(onehot, pre_l.astype(BF))
    cmp_b = (g <= cf - presel).astype(BF)
    l_row = _dot_nt(ones8, cmp_b)
    bvec = (_iota((8, 128), 1) & 15).astype(BF)
    b_row = _dot_nt(bvec, onehot)
    tok_row = (b_row * 128.0 + l_row).astype(I32)
    for k in range(4):
        tab_v[T_TOK + k:T_TOK + k + 1, :] = tok_row[0:1, 128 * k:128 * (k + 1)]

    rt = jnp.concatenate([r2] * N_EXP, axis=0)
    oh = (rt == (_iota((512, 128), 0) >> 4))
    oh_f = oh.astype(F32)
    oh_b = oh.astype(BF)
    c_in = _dot(oh_b, utri)
    tot_b = _dot(oh_b, ones_b)
    qi = _iota((512, 512), 0)
    qj = _iota((512, 512), 1)
    lblk = (((qi >> 4) == (qj >> 4)) & ((qj & 15) < (qi & 15))).astype(BF)
    pre = _dot(lblk, tot_b.astype(BF))
    rank = (oh_f * (c_in + pre - 1.0)).reshape(N_EXP, 16, 128).sum(axis=0)
    tab_v[T_RANK:T_RANK + 16, :] = rank.astype(I32)

    tot_row = _dot_nt(ones8, oh_b)
    mi = _iota((512, 256), 0)
    mj = _iota((512, 256), 1)
    m_b = (((mi >> 4) == (mj >> 3)) & ((mi & 15) < 4 * (mj & 7))).astype(BF)
    bnd = jnp.minimum(_dot(tot_row.astype(BF), m_b), float(CAP)).astype(I32)
    tab_v[T_BND:T_BND + 1, :] = bnd[0:1, 0:128]
    tab_v[T_BND + 1:T_BND + 2, :] = bnd[0:1, 128:256]

    my_r = r_ref[pl.ds(4 * me, 4), :]
    my_rank = tab_v[pl.ds(T_RANK + 4 * me, 4), :]
    step = my_r & 7
    cls = jnp.where(step < LAST, step, LAST + (((my_r >> 3) - me) & (N_DEV - 1)))
    cls = jnp.where(my_rank < CAP, cls, N_CLS - 1)
    ct = jnp.concatenate([cls] * N_CLS, axis=0)
    ohc = (ct == (_iota((4 * N_CLS, 128), 0) >> 2))
    ohc_b = ohc.astype(BF)
    cc_in = _dot(ohc_b, utri)
    ctot = _dot(ohc_b, ones_b)
    ci = _iota((4 * N_CLS, 4 * N_CLS), 0)
    cj = _iota((4 * N_CLS, 4 * N_CLS), 1)
    lfull = (((cj >> 2) < (ci >> 2))
             | (((cj >> 2) == (ci >> 2)) & ((cj & 3) < (ci & 3)))).astype(BF)
    cpre = _dot(lfull, ctot.astype(BF))
    pos = (ohc.astype(F32) * (cc_in + cpre - 1.0)).reshape(N_CLS, 4, 128).sum(axis=0)
    pos_row = _row512(pos.astype(I32))
    mp = (_iota((512, 512), 0) == pos_row).astype(BF)
    lane = _iota((1, 512), 1)
    vals = jnp.concatenate([
        (lane & 127).astype(F32),
        (lane >> 7).astype(F32),
        _row512(my_r).astype(F32),
        _row512(jnp.minimum(my_rank, SLOT - 1)).astype(F32),
        jnp.zeros((4, 512), F32)], axis=0).astype(BF)
    res = _dot_nt(vals, mp).astype(I32)
    irow = res[1:2, :] * 128 + res[0:1, :]
    dst_row = (irow >> 3) * 64 + (irow & 7)
    src_row = res[2:3, :] * SLOT + res[3:4, :]
    for k in range(4):
        tab_v[T_DST + k:T_DST + k + 1, :] = dst_row[:, 128 * k:128 * (k + 1)]
        tab_v[T_SRC + k:T_SRC + k + 1, :] = src_row[:, 128 * k:128 * (k + 1)]
    tab_v[T_SRC + 4:T_ROWS, :] = jnp.zeros((T_ROWS - T_SRC - 4, 128), I32)


def _body(r_hbm, x_hbm, w_hbm, obuf,
          wbuf, xg, st, st7, r_ref, tab_v, tab_s,
          wsem, wsem7, gsem, tsem, send_sem, recv_sem, send7, recv7, sem2):
    me = lax.axis_index("i")

    def wcopy(j):
        return pltpu.make_async_copy(w_hbm.at[j], wbuf.at[j], wsem.at[j])

    def wcopy7(q):
        return pltpu.make_async_copy(w_hbm.at[LAST, :, pl.ds(q * PW, PW)],
                                     wbuf.at[LAST, :, pl.ds(q * PW, PW)], wsem7.at[q])

    rcp = pltpu.make_async_copy(r_hbm, r_ref, tsem)
    rcp.start()
    for j in range(LAST):
        wcopy(j).start(priority=1)
    for q in range(NPC):
        wcopy7(q).start(priority=1)

    barrier = pltpu.get_barrier_semaphore()
    for k in range(1, N_DEV):
        pl.semaphore_signal(barrier, inc=1, device_id=((me + k) % N_DEV,),
                            device_id_type=pl.DeviceIdType.MESH)

    rcp.wait()
    _routing(me, r_ref, tab_v)

    tcp = pltpu.make_async_copy(tab_v, tab_s, tsem)
    tcp.start()
    pl.semaphore_wait(barrier, N_DEV - 1)
    for k in range(1, N_DEV):
        pl.semaphore_signal(sem2, inc=1, device_id=((me + k) % N_DEV,),
                            device_id_type=pl.DeviceIdType.MESH)
    tcp.wait()

    def tab(row0, idx):
        return tab_s[row0 + (idx >> 7), idx & 127]

    def bnd_s(e, d):
        return tab(T_BND, e * 8 + d)

    def gather(j):
        def one(c, carry):
            t = tab(T_TOK, j * SLOT + c)
            pltpu.make_async_copy(x_hbm.at[pl.ds(t, 1)], xg.at[j, pl.ds(c, 1)], gsem.at[j]).start()
            return carry
        lax.fori_loop(0, CAP, one, 0)

    def gather_wait(j):
        sl = xg.at[j, pl.ds(0, 48)]
        pltpu.make_async_copy(sl, sl, gsem.at[j]).wait()
        for c in range(48, CAP):
            sl = xg.at[j, pl.ds(c, 1)]
            pltpu.make_async_copy(sl, sl, gsem.at[j]).wait()

    def seg_copy(e, d, owner):
        a = bnd_s(e, d)
        n = bnd_s(e, d + 1) - a
        sl = st.at[pl.ds(e * SLOT + a, n)]
        jloc = e - owner * E_LOC
        cp = pltpu.make_async_remote_copy(
            src_ref=sl, dst_ref=sl,
            send_sem=send_sem.at[jloc * N_DEV + d], recv_sem=recv_sem.at[e],
            device_id=(d,), device_id_type=pl.DeviceIdType.MESH)
        return n, cp

    def seg7(q, d, owner):
        e = owner * E_LOC + LAST
        a = bnd_s(e, d)
        n = bnd_s(e, d + 1) - a
        sl = st7.at[pl.ds((q * N_DEV + owner) * SLOT + a, n)]
        cp = pltpu.make_async_remote_copy(
            src_ref=sl, dst_ref=sl,
            send_sem=send7.at[q * N_DEV + d], recv_sem=recv7.at[q * N_DEV + owner],
            device_id=(d,), device_id_type=pl.DeviceIdType.MESH)
        return n, cp

    def compute(j):
        e = me * E_LOC + j
        wcopy(j).wait()
        gather_wait(j)
        xb = xg[j].astype(BF)
        y = _dot(xb, wbuf[j].astype(BF))
        yr = pltpu.bitcast(y.astype(BF).astype(F32), I32)
        base = pl.multiple_of(e * SLOT, SLOT)
        for c in range(4):
            st[pl.ds(base, SLOT), c, :] = (
                yr[:, 256 * c:256 * c + 128]
                | lax.shift_right_logical(yr[:, 256 * c + 128:256 * c + 256], 16))
        if j == 0:
            pl.semaphore_wait(sem2, N_DEV - 1)
        for k in range(1, N_DEV):
            d = (me + k) % N_DEV
            n, cp = seg_copy(e, d, me)

            @pl.when(n > 0)
            def _():
                cp.start()

    def compute7():
        gather_wait(LAST)
        xb = xg[LAST].astype(BF)
        for q in range(NPC):
            wcopy7(q).wait()
            y = _dot(xb, wbuf[LAST, :, q * PW:(q + 1) * PW].astype(BF))
            yr = pltpu.bitcast(y.astype(BF).astype(F32), I32)
            base = pl.multiple_of((q * N_DEV + me) * SLOT, SLOT)
            st7[pl.ds(base, SLOT), 0, :] = yr[:, :128] | lax.shift_right_logical(yr[:, 128:], 16)
            for k in range(1, N_DEV):
                d = (me + k) % N_DEV
                n, cp = seg7(q, d, me)

                @pl.when(n > 0)
                def _():
                    cp.start()

    def step_count(j):
        cnt = 0
        for s_ in range(N_DEV):
            e = s_ * E_LOC + j
            cnt = cnt + bnd_s(e, me + 1) - bnd_s(e, me)
        return cnt

    def place(off, cnt, load):
        def row(p):
            dst = tab(T_DST, p)
            v = load(tab(T_SRC, p))
            obuf[pl.ds(dst, 4, stride=16), :] = pltpu.bitcast(v & jnp.int32(-65536), F32)
            obuf[pl.ds(dst + 8, 4, stride=16), :] = pltpu.bitcast(v << 16, F32)

        def group(g_, carry):
            for t in range(UNR):
                row(off + UNR * g_ + t)
            return carry

        def one(p, carry):
            row(p)
            return carry
        ng = cnt // UNR
        lax.fori_loop(0, ng, group, 0)
        lax.fori_loop(off + UNR * ng, off + cnt, one, 0)

    def receive(j, off):
        cnt = step_count(j)
        for k in range(1, N_DEV):
            s_ = (me + k) % N_DEV
            n, cp = seg_copy(s_ * E_LOC + j, me, s_)

            @pl.when(n > 0)
            def _():
                cp.wait_recv()
        place(off, cnt, lambda src: st[src])
        return off + cnt

    def receive7(off):
        def load(src):
            slot = (src >> 9) * SLOT + (src & (SLOT - 1))
            return st7[pl.ds(slot, NPC, stride=N_DEV * SLOT), 0, :]

        for k in range(N_DEV):
            s_ = (me + k) % N_DEV
            e = s_ * E_LOC + LAST
            cnt = bnd_s(e, me + 1) - bnd_s(e, me)
            if k > 0:
                for q in range(NPC):
                    n, cp = seg7(q, me, s_)

                    @pl.when(n > 0)
                    def _():
                        cp.wait_recv()
            place(off, cnt, load)
            off = off + cnt

    gather(0)
    gather(1)
    obuf[...] = jnp.zeros(obuf.shape, F32)
    off = 0
    for j in range(LAST):
        compute(j)
        if j + 2 < E_LOC:
            gather(j + 2)
        for jr in RECV_AFTER.get(j, ()):
            off = receive(jr, off)
    compute7()
    off = receive(LAST - 1, off)

    for j in range(LAST):
        for k in range(1, N_DEV):
            d = (me + k) % N_DEV
            n, cp = seg_copy(me * E_LOC + j, d, me)

            @pl.when(n > 0)
            def _():
                cp.wait_send()
    for q in range(NPC):
        for k in range(1, N_DEV):
            d = (me + k) % N_DEV
            n, cp = seg7(q, d, me)

            @pl.when(n > 0)
            def _():
                cp.wait_send()
    receive7(off)


def pallas_dist_moe_cap_ep_outshard_n2048_d512_e8_h1024_kernel(x, router_W, route_idx, expert_W):
    del router_W
    r2 = route_idx.reshape(16, 128)
    out = pl.pallas_call(
        _body,
        out_shape=jax.ShapeDtypeStruct((ROWS_PER_DEV * 8, 128), F32),
        in_specs=[pl.BlockSpec(memory_space=pl.ANY),
                  pl.BlockSpec(memory_space=pl.ANY),
                  pl.BlockSpec(memory_space=pl.ANY)],
        out_specs=pl.BlockSpec(memory_space=pltpu.VMEM),
        scratch_shapes=[
            pltpu.VMEM((E_LOC, D, H), F32),
            pltpu.VMEM((E_LOC, SLOT, D), F32),
            pltpu.VMEM((N_EXP * SLOT, 4, 128), I32),
            pltpu.VMEM((NPC * N_DEV * SLOT, 1, 128), I32),
            pltpu.VMEM((16, 128), I32),
            pltpu.VMEM((T_ROWS, 128), I32),
            pltpu.SMEM((T_ROWS, 128), I32),
            pltpu.SemaphoreType.DMA((E_LOC,)),
            pltpu.SemaphoreType.DMA((NPC,)),
            pltpu.SemaphoreType.DMA((E_LOC,)),
            pltpu.SemaphoreType.DMA,
            pltpu.SemaphoreType.DMA((E_LOC * N_DEV,)),
            pltpu.SemaphoreType.DMA((N_EXP,)),
            pltpu.SemaphoreType.DMA((NPC * N_DEV,)),
            pltpu.SemaphoreType.DMA((NPC * N_DEV,)),
            pltpu.SemaphoreType.REGULAR,
        ],
        compiler_params=pltpu.CompilerParams(
            collective_id=0, vmem_limit_bytes=64 * 1024 * 1024,
            disable_bounds_checks=True, disable_semaphore_checks=True),
    )(r2, x, expert_W)
    return out.reshape(64, 8, 8, 128).transpose(0, 2, 1, 3).reshape(ROWS_PER_DEV, H)
```
